```python
import numpy as np

kernel_name = "dist_pipemlp_pp2tp2_xy_b4096_d256_h512"

def setup_inputs():
    x_padded = np.zeros((2, 4096, 256), dtype=np.float32)
    x_padded[0] = np.random.randn(4096, 256).astype(np.float32)
    Win = np.random.randn(4, 256, 1024).astype(np.float32)
    Wout = np.random.randn(4, 1024, 256).astype(np.float32)
    return {"x_padded": x_padded, "Win": Win, "Wout": Wout}

def reference(x_padded, Win, Wout):
    a = x_padded[0]
    for k in range(4):
        h = a @ Win[k]
        h = np.maximum(h, 0.0)
        a = h @ Wout[k]
    out = np.zeros_like(x_padded)
    out[1] = a
    return out
```

```python
import contextlib

import jax
import jax.numpy as jnp
from jax import lax
from jax.experimental import pallas as pl
from jax.experimental.pallas import tpu as pltpu

F32 = jnp.float32
BF16 = jnp.bfloat16
MESH = pl.DeviceIdType.MESH

ROWS = 4096
D = 256
HL = 512
HALF = ROWS // 2
WIN, WOUT = 0, 1

CFG = dict(
    c=64,
    far=(13, 16),
    piece0=64,
    last_cuts=(0, 256, 512),
    xload=4,
    q_first=(8,),
    q_runs=((7, 3), (5, 2)),
    fwd0=27,
    late=8,
    phase1=(("new", 5, 2, 512), ("more", 0, 6, 768), ("swap", 2), ("more", 6, 4, 768),
            ("new", 2, 2, 768), ("new", 1, 2, 0)),
    phase2=((1, 2, 12, 2), (1, 2, 14, 2), (1, 10, 0, 6), (1, 2, 16, 0)),
    phase3=((1, 4, 0), (4, 2, 2), (2, 1, 1)),
)


def _make_body(cfg):
    c = cfg["c"]
    nc = HALF // c
    fwd0 = cfg["fwd0"]
    n_far, far_rows = cfg["far"]
    far = n_far * far_rows
    (nq,) = [step[1] for step in cfg["phase1"] if step[0] == "swap"]
    nfin = nc - nq
    detour = []
    base = 0
    for groups, n, n_direct in [(g, n, d) for g, n, _, d in cfg["phase2"]] + list(cfg["phase3"]):
        detour += [base + g * n + t for g in range(groups) for t in range(n_direct, n)]
        base += groups * n
    ndet = len(detour)
    det0 = detour[0] if detour else 0
    assert detour == list(range(det0, det0 + ndet))

    def scope(name):
        if cfg.get("trace"):
            return jax.named_scope("s_" + name)
        return contextlib.nullcontext()

    def body(x_hbm, win_hbm, wout_hbm, out_ref,
             win_f, wout_f, win, wout, xs, acc, part_s, part_r, act, fin_s, fin_r, relay,
             w_sem, x_sem, send_sems, w_rsem, part_rsem, act_rsem, fin_rsem, far_rsem, entered):
        mx = lax.axis_index("x")
        my = lax.axis_index("y")
        x_nbr = (1 - mx, my)
        y_nbr = (mx, 1 - my)
        own0 = pl.multiple_of(my * HALF, HALF)
        oth0 = pl.multiple_of((1 - my) * HALF, HALF)

        barrier = pltpu.get_barrier_semaphore()

        def signal(sem, dev):
            pl.semaphore_signal(sem, 1, device_id=dev, device_id_type=MESH)

        signal(barrier, y_nbr)
        pl.when((mx == 1) & (my == 0))(lambda: signal(barrier, x_nbr))

        def rows(k, n=1):
            start = k * c
            return pl.ds(start if isinstance(k, int) else pl.multiple_of(start, c), n * c)

        def loop(n, fn):
            if n == 1:
                fn(0)
            elif n > 1:
                lax.fori_loop(0, n, lambda i, _: fn(i), None)

        def remote(src, dst, send_sem, recv_sem, dev):
            return pltpu.make_async_remote_copy(
                src, dst, send_sem, recv_sem, device_id=dev, device_id_type=MESH)

        def w_view(refs, layer, piece, shift=0):
            m, h0, n = piece
            hid = pl.ds(h0 + shift, n)
            return refs[m].at[layer, :, hid] if m == WIN else refs[m].at[layer, hid, :]

        class Piece:
            def __init__(self, i, layer, piece):
                self.i, self.layer, self.piece = i, layer, piece

            def view(self, refs, shift=0):
                return w_view(refs, self.layer, self.piece, shift)

            def load(self):
                return pltpu.make_async_copy(
                    self.view((win_hbm, wout_hbm)), self.view((win_f, wout_f)), w_sem.at[self.i])

            def cast(self):
                with scope(f"ld{self.i}"):
                    self.load().wait()
                self.view((win, wout))[...] = self.view((win_f, wout_f))[...].astype(BF16)

            def swap(self):
                return remote(self.view((win, wout)), self.view((win, wout), HL),
                              send_sems.at[0], w_rsem.at[self.i], y_nbr)

        def far_hop(hop, i):
            r0 = i * far_rows
            here = pl.ds(r0, far_rows)
            src = wout.at[1, pl.ds(HL - far + r0, far_rows)] if hop == 0 else relay.at[hop - 1, here]
            dst = wout.at[1, pl.ds(2 * HL - far + r0, far_rows)] if hop == 2 else relay.at[hop, here]
            return remote(src, dst, send_sems.at[5], far_rsem.at[hop * n_far + i],
                          y_nbr if hop == 1 else x_nbr)

        def far_start():
            for i in range(n_far):
                far_hop(0, i).start()

        def part_copy(k):
            return remote(part_s.at[rows(k)], part_r.at[rows(k)], send_sems.at[1],
                          part_rsem.at[k], y_nbr)

        def act_copy(k):
            return remote(act.at[rows(k)], act.at[rows(k)], send_sems.at[2],
                          act_rsem.at[k], x_nbr)

        def fin_copy(j):
            return remote(fin_s.at[rows(j)], fin_r.at[rows(j)], send_sems.at[3],
                          fin_rsem.at[j], y_nbr)

        def detour_in(j):
            return remote(fin_s.at[rows(j)], fin_s.at[rows(j)], send_sems.at[4],
                          act_rsem.at[j], x_nbr)

        def detour_out(j):
            return remote(fin_r.at[rows(j)], fin_r.at[rows(j)], send_sems.at[4],
                          fin_rsem.at[j], x_nbr)

        def mlp(a, layer, h0=0, h1=2 * HL):
            h = jnp.dot(a, win[layer, :, h0:h1], preferred_element_type=F32)
            h = jnp.maximum(h, 0.0).astype(BF16)
            return jnp.dot(h, wout[layer, h0:h1, :], preferred_element_type=F32)

        @pl.when(mx == 0)
        def _stage0():
            p0 = cfg["piece0"]
            shared = ((WOUT, 0, p0), (WOUT, p0, HL - far - p0), (WIN, 0, 128), (WIN, 128, HL - 128))
            shared = [Piece(i, 1, p) for i, p in enumerate(shared)]
            local = [Piece(len(shared) + m, 0, (m, 0, HL)) for m in (WIN, WOUT)]
            far_piece = Piece(len(shared) + 2, 1, (WOUT, HL - far, far))
            xn = cfg["xload"]

            def x_load(i):
                src = pl.multiple_of((oth0 + i * xn * c) % ROWS, xn * c)
                return pltpu.make_async_copy(
                    x_hbm.at[0, pl.ds(src, xn * c)], xs.at[rows(i * xn, xn)], x_sem.at[i])

            def x_get(k, n, ahead=None):
                for t in range(n // xn):
                    i = k // xn + t
                    with scope("x"):
                        x_load(i).wait()
                    if ahead:
                        x_load(i + ahead).start()
                return xs[rows(k, n), :].astype(BF16)

            def nbr_partial(k, n, ahead):
                part_s[rows(k, n), :] = mlp(x_get(k, n, ahead), 0, 0, HL).astype(BF16)

            for s in shared[:2]:
                s.load().start()
            shared[0].cast()
            for s in local:
                s.load().start()
            x_load(0).start()
            with scope("bar"):
                pl.when(my == 0)(lambda: pl.semaphore_wait(barrier, 2))
                pl.when(my == 1)(lambda: pl.semaphore_wait(barrier, 1))
            shared[0].swap().start()
            pl.when(my == 0)(lambda: signal(entered, x_nbr))
            shared[1].cast()
            shared[1].swap().start()
            local[0].cast()
            far_piece.load().start()
            shared[2].load().start()
            local[1].cast()
            far_piece.cast()
            pl.when(my == 0)(far_start)
            with scope("ent"):
                pl.semaphore_wait(entered, 1)
            pl.when(my == 0)(lambda: signal(entered, y_nbr))
            pl.when(my == 1)(far_start)
            shared[2].cast()
            shared[2].swap().start()
            shared[3].load().start()
            x_load(1).start()

            nbr_partial(0, xn, 2)
            shared[3].cast()
            shared[3].swap().start()

            def part_start(k0, n):
                for t in range(n):
                    part_copy(k0 + t).start()

            part_start(0, xn)
            nbr_partial(xn, xn, 2)
            part_start(xn, xn)
            x_load(4).start()
            x_load(5).start()

            def nbr_step(i):
                k0 = 2 * xn * (i + 1)
                nbr_partial(k0, 2 * xn, 4)
                part_start(k0, 2 * xn)

            loop(nc // (2 * xn) - 1, nbr_step)

            for i in range(nc // xn + 4, 2 * nc // xn):
                x_load(i).start()
            done = 0
            for n in cfg["q_first"]:
                acc[rows(done, n), :] = mlp(x_get(nc + done, n), 0, 0, HL)
                done += n
            for i in range((nc + done) // xn, 2 * nc // xn):
                x_load(i).wait()

            with scope("w1"):
                for s in shared:
                    s.swap().wait_recv()
                for i in range(n_far):
                    far_hop(2, i).wait_recv()

            def forward(j):
                with scope("d"):
                    detour_in(j).wait_recv()
                fin_copy(j).start()

            def stream_step(k, more=None):
                with scope("p"):
                    part_copy(k).wait_recv()
                a1 = (acc[rows(k), :] + part_r[rows(k), :].astype(F32)).astype(BF16)
                act[rows(k), :] = mlp(a1, 1).astype(BF16)
                act_copy(k).start()
                if more is not None:
                    x = xs[rows(nc + more, 2), :].astype(BF16)
                    acc[rows(more, 2), :] = mlp(x, 0, 0, HL)
                out_ref[0, rows(2 * k, 2), :] = jnp.zeros((2 * c, D), F32)
                pl.when((k >= fwd0) & (k < fwd0 + ndet))(lambda: forward(det0 + k - fwd0))

            k0 = 0
            for runs, length in cfg["q_runs"]:
                assert all(k0 + i * length < done + 2 * i for i in range(runs))

                def stream_run(i, k0=k0, done=done, length=length):
                    stream_step(k0 + i * length, more=done + 2 * i)
                    loop(length - 1, lambda t: stream_step(k0 + i * length + 1 + t))

                loop(runs, stream_run)
                k0 += runs * length
                done += 2 * runs
            assert done == nc and k0 <= nc
            loop(nc - k0, lambda k: stream_step(k0 + k))
            for s in shared:
                s.swap().wait_send()
            for i in range(n_far):
                far_hop(0, i).wait_send()
            for k in range(nc):
                part_copy(k).wait_send()
            for j in detour:
                if j + nc - fwd0 in detour:
                    forward(j + nc - fwd0)
                with scope("h"):
                    fin_copy(j).wait_recv()
                detour_out(j).start()

            with scope("end"):
                for k in range(nc):
                    act_copy(k).wait_send()
                for j in detour:
                    fin_copy(j).wait_send()
                for j in detour:
                    detour_out(j).wait_send()

        @pl.when(mx == 1)
        def _stage1():
            p0 = cfg["piece0"]
            first = ((WOUT, 0, p0), (WOUT, p0, 384 - p0), (WOUT, 384, HL - 384), (WIN, 0, HL))
            first = [Piece(i, 0, p) for i, p in enumerate(first)]
            cuts = cfg["last_cuts"]
            last = [(m, a, b - a) for a, b in zip(cuts, cuts[1:]) for m in (WIN, WOUT)]
            last = [Piece(len(first) + i, 1, p) for i, p in enumerate(last)]
            pieces = first + last
            first[0].load().start()
            first[1].load().start()
            first[0].cast()
            with scope("bar"):
                pl.semaphore_wait(barrier, 1)
            first[0].swap().start()
            first[1].cast()
            first[1].swap().start()

            @pl.when(my == 0)
            def _():
                pl.semaphore_wait(entered, 1)
                signal(entered, x_nbr)

            for s in first[2:]:
                s.load().start()
            for i in range(n_far):
                with scope("far0"):
                    far_hop(0, i).wait_recv()
                far_hop(1, i).start()
            for s in first[2:]:
                s.cast()
                s.swap().start()
            for s in last:
                s.load().start()
            for i in range(n_far):
                with scope("far1"):
                    far_hop(1, i).wait_recv()
                far_hop(2, i).start()
            for s in last:
                s.cast()
                s.swap().start()

            n_early = nq + sum(groups * n for groups, n, _, _ in cfg["phase2"])

            chunk_at = [k0 + t for groups, n, k0, _ in cfg["phase2"] for t in range(groups * n)]
            chunk_at += range(n_early, nc)

            def finish(j0, k0, n, n_direct, val):
                fin_s[rows(j0, n), :] = val.astype(BF16)
                for t in range(n):
                    (fin_copy if t < n_direct else detour_in)(j0 + t).start()
                out_ref[0, pl.ds(pl.multiple_of(own0 + k0 * c, c), n * c), :] = val

            def layer2(k0, n):
                with scope("a"):
                    for t in range(n):
                        act_copy(k0 + t).wait_recv()
                return mlp(act[rows(k0, n), :], 0).astype(BF16)

            pending = list(last)

            def need(h):
                with scope(f"w3_{h}"):
                    while pending and HL + pending[0].piece[1] < h:
                        pending.pop(0).swap().wait_recv()

            with scope("w2"):
                for s in first:
                    s.swap().wait_recv()

            covered = []
            for kind, *step in cfg["phase1"]:
                base = len(covered)
                if kind == "swap":
                    q0 = base
                    part_s[rows(q0, nq), :] = layer2(q0, nq)
                    for k in range(q0, q0 + nq):
                        part_copy(k).start()
                    covered += [None] * nq
                elif kind == "new":
                    groups, n, h = step
                    need(h)

                    def early_step(i, base=base, n=n, h=h):
                        k0 = base + i * n
                        a3 = layer2(k0, n)
                        part_s[rows(k0, n), :] = a3
                        if h:
                            acc[rows(k0, n), :] = mlp(a3, 1, 0, h)

                    loop(groups, early_step)
                    covered += [h] * (groups * n)
                else:
                    k0, n, h = step
                    (h0,) = set(covered[k0:k0 + n])
                    need(h)
                    acc[rows(k0, n), :] += mlp(part_s[rows(k0, n), :], 1, h0, h)
                    covered[k0:k0 + n] = [h] * n
            assert sorted(chunk_at[:n_early - nq]) == [
                k for k, h in enumerate(covered) if h is not None]
            need(2 * HL)
            base = 0
            for groups, n, k_base, n_direct in cfg["phase2"]:
                (h,) = set(covered[k_base:k_base + groups * n])

                def late_step(i, base=base, k_base=k_base, n=n, h=h, n_direct=n_direct):
                    r = rows(k_base + i * n, n)
                    val = mlp(part_s[r, :], 1, h)
                    finish(base + i * n, k_base + i * n, n, n_direct, acc[r, :] + val if h else val)

                loop(groups, late_step)
                base += groups * n
            assert nq + base == n_early
            for groups, n, n_direct in cfg["phase3"]:
                def full_step(i, base=base, n=n, n_direct=n_direct):
                    j0 = base + i * n
                    finish(j0, nq + j0, n, n_direct, mlp(layer2(nq + j0, n), 1))

                loop(groups, full_step)
                base += groups * n
            assert base == nfin

            direct = [j for j in range(nfin) if j not in detour]
            round_trip = list(detour)
            order = []
            while direct or round_trip:
                for queue in (direct, round_trip):
                    if queue:
                        order.insert(0, queue.pop())

            def land(j):
                dst = pl.ds(pl.multiple_of(oth0 + chunk_at[j] * c, c), c)
                out_ref[0, dst, :] = fin_r[rows(j), :].astype(F32)

            here, late = order[:-cfg["late"]], order[-cfg["late"]:]
            with scope("q"):
                for k in range(q0, q0 + nq):
                    part_copy(k).wait_recv()
                for j in here:
                    fin_copy(j).wait_recv()
            both = mlp(jnp.concatenate([part_s[rows(q0, nq), :], part_r[rows(q0, nq), :]]), 1)
            out_ref[0, pl.ds(pl.multiple_of(own0 + q0 * c, c), nq * c), :] = both[:nq * c]
            out_ref[0, pl.ds(pl.multiple_of(oth0 + q0 * c, c), nq * c), :] = both[nq * c:]
            for j in here:
                land(j)
            with scope("end"):
                for s in pieces:
                    s.swap().wait_send()
                for i in range(n_far):
                    far_hop(1, i).wait_send()
                    far_hop(2, i).wait_send()
                for k in range(nq):
                    part_copy(k).wait_send()
                for j in range(nfin):
                    (detour_in if j in detour else fin_copy)(j).wait_send()
            for j in late:
                with scope(f"l{j}"):
                    fin_copy(j).wait_recv()
                land(j)

    return body


def _build(cfg):
    nc = HALF // cfg["c"]
    n_w = 4 + 2 * (len(cfg["last_cuts"]) - 1)
    n_x = 2 * nc // cfg["xload"]
    dma = pltpu.SemaphoreType.DMA
    hbm = pl.BlockSpec(memory_space=pltpu.HBM)
    return pl.pallas_call(
        _make_body(cfg),
        out_shape=jax.ShapeDtypeStruct((1, ROWS, D), F32),
        in_specs=[hbm, hbm, hbm],
        out_specs=pl.BlockSpec(memory_space=pltpu.VMEM),
        scratch_shapes=[
            pltpu.VMEM((2, D, HL), F32),
            pltpu.VMEM((2, HL, D), F32),
            pltpu.VMEM((2, D, 2 * HL), BF16),
            pltpu.VMEM((2, 2 * HL, D), BF16),
            pltpu.VMEM((ROWS, D), F32),
            pltpu.VMEM((HALF, D), F32),
            pltpu.VMEM((HALF, D), BF16),
            pltpu.VMEM((HALF, D), BF16),
            pltpu.VMEM((HALF, D), BF16),
            pltpu.VMEM((HALF, D), BF16),
            pltpu.VMEM((HALF, D), BF16),
            pltpu.VMEM((2, cfg["far"][0] * cfg["far"][1], D), BF16),
            dma((n_w,)),
            dma((n_x,)),
            dma((6,)),
            dma((n_w,)),
            dma((nc,)),
            dma((nc,)),
            dma((nc,)),
            dma((3 * cfg["far"][0],)),
            pltpu.SemaphoreType.REGULAR,
        ],
        compiler_params=pltpu.CompilerParams(
            collective_id=0, vmem_limit_bytes=64 * 1024 * 1024,
            disable_semaphore_checks=not cfg.get("check_sems"), **cfg.get("cp", {})),
    )


def pallas_dist_pipemlp_pp2tp2_xy_b4096_d256_h512_kernel(
    x_padded: jax.Array,
    Win: jax.Array,
    Wout: jax.Array,
):
    return _build(CFG)(x_padded, Win, Wout)
```

```python
import jax
import jax.numpy as jnp
from jax import lax
from jax.experimental import pallas as pl
from jax.experimental.pallas import tpu as pltpu

F32 = jnp.float32
BF16 = jnp.bfloat16
MESH = pl.DeviceIdType.MESH

ROWS = 4096
D = 256
HL = 512
HALF = ROWS // 2
C = 64
NC = HALF // C
WIN, WOUT = 0, 1

RELAY = (48, 64, 48, 32, 32)
N_RELAY = sum(RELAY)
LAYER1_PIECES = ((WOUT, 0, 64), (WOUT, 64, HL - N_RELAY - 64), (WIN, 0, 128), (WIN, 128, HL - 128))
LAYER2_PIECES = ((WOUT, 0, 64), (WOUT, 64, 320), (WOUT, 384, 128), (WIN, 0, HL))
LAYER3_PIECES = ((WIN, 0, 256), (WOUT, 0, 256), (WIN, 256, 256), (WOUT, 256, 256))

XN = 4
OWN_FIRST = 8
OWN_LATER = ((7, 3), (5, 2))
FORWARD_FROM = 27

EARLY = (("new", 5, 2, HL), ("more", 0, 10, HL + 256), ("swap", 2),
         ("new", 2, 2, HL + 256), ("new", 1, 2, 0))
FINISH = ((12, 2, 2), (14, 2, 2), (0, 10, 6), (16, 2, 0))
STEADY = ((1, 4, 0), (4, 2, 2), (2, 1, 1))

N_SWAP = sum(step[1] for step in EARLY if step[0] == "swap")
N_SENT = NC - N_SWAP
CHUNK_AT = [k + t for k, n, _ in FINISH for t in range(n)]
CHUNK_AT += range(N_SWAP + len(CHUNK_AT), NC)
_STRAIGHT = [t < s for _, n, s in FINISH for t in range(n)]
_STRAIGHT += [t < s for groups, n, s in STEADY for _ in range(groups) for t in range(n)]
DETOUR = [j for j in range(N_SENT) if not _STRAIGHT[j]]
assert len(_STRAIGHT) == N_SENT and DETOUR == list(range(DETOUR[0], DETOUR[-1] + 1))
N_LATE = 8


def _arrival_order():
    queues = [[j for j in range(N_SENT) if _STRAIGHT[j]], list(DETOUR)]
    order = []
    while any(queues):
        for queue in queues:
            if queue:
                order.insert(0, queue.pop())
    return order


def _rows(k, n=1):
    start = k * C
    return pl.ds(start if isinstance(k, int) else pl.multiple_of(start, C), n * C)


def _loop(n, fn):
    if n == 1:
        fn(0)
    elif n > 1:
        lax.fori_loop(0, n, lambda i, _: fn(i), None)


def _body(x_hbm, win_hbm, wout_hbm, out_ref,
          win_f, wout_f, win, wout, xs, acc, part_s, part_r, act, fin_s, fin_r, relay,
          w_sem, x_sem, send_sems, w_rsem, part_rsem, act_rsem, fin_rsem, relay_rsem, entered):
    mx = lax.axis_index("x")
    my = lax.axis_index("y")
    x_nbr = (1 - mx, my)
    y_nbr = (mx, 1 - my)

    def own_out(k, n=1):
        return pl.ds(pl.multiple_of(my * HALF + k * C, C), n * C)

    def nbr_out(k, n=1):
        return pl.ds(pl.multiple_of((1 - my) * HALF + k * C, C), n * C)

    def signal(sem, dev):
        pl.semaphore_signal(sem, 1, device_id=dev, device_id_type=MESH)

    barrier = pltpu.get_barrier_semaphore()
    signal(barrier, y_nbr)
    pl.when((mx == 1) & (my == 0))(lambda: signal(barrier, x_nbr))

    def remote(src, dst, send_sem, recv_sem, dev):
        return pltpu.make_async_remote_copy(
            src, dst, send_sem, recv_sem, device_id=dev, device_id_type=MESH)

    class Piece:
        def __init__(self, i, layer, piece):
            self.i, self.layer, self.piece = i, layer, piece

        def view(self, refs, shift=0):
            m, h0, n = self.piece
            hidden = pl.ds(h0 + shift, n)
            if m == WIN:
                return refs[m].at[self.layer, :, hidden]
            return refs[m].at[self.layer, hidden, :]

        def load(self):
            return pltpu.make_async_copy(
                self.view((win_hbm, wout_hbm)), self.view((win_f, wout_f)), w_sem.at[self.i])

        def cast(self):
            self.load().wait()
            self.view((win, wout))[...] = self.view((win_f, wout_f))[...].astype(BF16)

        def send(self):
            return remote(self.view((win, wout)), self.view((win, wout), HL),
                          send_sems.at[0], w_rsem.at[self.i], y_nbr)

    def relay_copy(hop, i):
        r0, n = sum(RELAY[:i]), RELAY[i]
        here = pl.ds(r0, n)
        src = wout.at[1, pl.ds(HL - N_RELAY + r0, n)] if hop == 0 else relay.at[hop - 1, here]
        dst = wout.at[1, pl.ds(2 * HL - N_RELAY + r0, n)] if hop == 2 else relay.at[hop, here]
        return remote(src, dst, send_sems.at[5], relay_rsem.at[hop * len(RELAY) + i],
                      y_nbr if hop == 1 else x_nbr)

    def relay_each(y, fn):
        pl.when(y == 1)(lambda: fn(0))
        for i in range(1, len(RELAY)):
            fn(i)

    def relay_direct():
        h0 = HL - N_RELAY
        return remote(wout.at[1, pl.ds(h0, RELAY[0])], wout.at[1, pl.ds(HL + h0, RELAY[0])],
                      send_sems.at[5], relay_rsem.at[0], y_nbr)

    def part_copy(k):
        return remote(part_s.at[_rows(k)], part_r.at[_rows(k)], send_sems.at[1],
                      part_rsem.at[k], y_nbr)

    def act_copy(k):
        return remote(act.at[_rows(k)], act.at[_rows(k)], send_sems.at[2], act_rsem.at[k], x_nbr)

    def fin_copy(j):
        return remote(fin_s.at[_rows(j)], fin_r.at[_rows(j)], send_sems.at[3],
                      fin_rsem.at[j], y_nbr)

    def detour_in(j):
        return remote(fin_s.at[_rows(j)], fin_s.at[_rows(j)], send_sems.at[4],
                      act_rsem.at[j], x_nbr)

    def detour_out(j):
        return remote(fin_r.at[_rows(j)], fin_r.at[_rows(j)], send_sems.at[4],
                      fin_rsem.at[j], x_nbr)

    def mlp(a, layer, h0=0, h1=2 * HL):
        h = jnp.dot(a, win[layer, :, h0:h1], preferred_element_type=F32)
        h = jnp.maximum(h, 0.0).astype(BF16)
        return jnp.dot(h, wout[layer, h0:h1, :], preferred_element_type=F32)

    @pl.when(mx == 0)
    def _stage0():
        shared = [Piece(i, 1, p) for i, p in enumerate(LAYER1_PIECES)]
        local = [Piece(len(shared) + m, 0, (m, 0, HL)) for m in (WIN, WOUT)]
        relayed = Piece(len(shared) + 2, 1, (WOUT, HL - N_RELAY, N_RELAY))

        def x_load(i):
            src = pl.multiple_of(((1 - my) * HALF + i * XN * C) % ROWS, XN * C)
            return pltpu.make_async_copy(
                x_hbm.at[0, pl.ds(src, XN * C)], xs.at[_rows(i * XN, XN)], x_sem.at[i])

        def layer0(k, n):
            return mlp(xs[_rows(k, n), :].astype(BF16), 0, 0, HL)

        def nbr_partial(i, loads, ahead):
            for t in range(loads):
                x_load(i + t).wait()
                x_load(i + t + ahead).start()
            part_s[_rows(i * XN, loads * XN), :] = layer0(i * XN, loads * XN).astype(BF16)

        def part_start(i, loads):
            for t in range(loads * XN):
                part_copy(i * XN + t).start()

        shared[0].load().start()
        shared[1].load().start()
        shared[0].cast()
        for s in local:
            s.load().start()
        x_load(0).start()
        pl.when(my == 0)(lambda: pl.semaphore_wait(barrier, 2))
        pl.when(my == 1)(lambda: pl.semaphore_wait(barrier, 1))
        shared[0].send().start()
        pl.when(my == 0)(lambda: signal(entered, x_nbr))
        shared[1].cast()
        shared[1].send().start()
        local[0].cast()
        relayed.load().start()
        shared[2].load().start()
        local[1].cast()
        relayed.cast()

        @pl.when(my == 0)
        def _():
            relay_direct().start()
            relay_each(0, lambda i: relay_copy(0, i).start())

        pl.semaphore_wait(entered, 1)
        pl.when(my == 0)(lambda: signal(entered, y_nbr))

        @pl.when(my == 1)
        def _():
            signal(entered, x_nbr)
            relay_each(1, lambda i: relay_copy(0, i).start())

        shared[2].cast()
        shared[2].send().start()
        shared[3].load().start()
        x_load(1).start()

        nbr_partial(0, 1, 2)
        shared[3].cast()
        shared[3].send().start()
        part_start(0, 1)
        nbr_partial(1, 1, 2)
        part_start(1, 1)
        x_load(4).start()
        x_load(5).start()

        def nbr_step(i):
            nbr_partial(2 * i + 2, 2, 4)
            part_start(2 * i + 2, 2)

        n_loads = NC // XN
        _loop(n_loads // 2 - 1, nbr_step)

        for i in range(n_loads + 4, 2 * n_loads):
            x_load(i).start()
        for i in range(n_loads, n_loads + OWN_FIRST // XN):
            x_load(i).wait()
        acc[_rows(0, OWN_FIRST), :] = layer0(NC, OWN_FIRST)
        for i in range(n_loads + OWN_FIRST // XN, 2 * n_loads):
            x_load(i).wait()

        for s in shared:
            s.send().wait_recv()
        relay_each(1 - my, lambda i: relay_copy(2, i).wait_recv())
        pl.when(my == 1)(lambda: relay_direct().wait_recv())

        def forward(j):
            detour_in(j).wait_recv()
            fin_copy(j).start()

        def stream_step(k, own=None):
            part_copy(k).wait_recv()
            a1 = (acc[_rows(k), :] + part_r[_rows(k), :].astype(F32)).astype(BF16)
            act[_rows(k), :] = mlp(a1, 1).astype(BF16)
            act_copy(k).start()
            if own is not None:
                acc[_rows(own, 2), :] = layer0(NC + own, 2)
            out_ref[0, _rows(2 * k, 2), :] = jnp.zeros((2 * C, D), F32)
            pl.when((k >= FORWARD_FROM) & (k < FORWARD_FROM + len(DETOUR)))(
                lambda: forward(DETOUR[0] + k - FORWARD_FROM))

        k0, done = 0, OWN_FIRST
        for runs, length in OWN_LATER:
            assert all(k0 + i * length < done + 2 * i for i in range(runs))

            def stream_run(i, k0=k0, done=done, length=length):
                stream_step(k0 + i * length, own=done + 2 * i)
                _loop(length - 1, lambda t: stream_step(k0 + i * length + 1 + t))

            _loop(runs, stream_run)
            k0, done = k0 + runs * length, done + 2 * runs
        assert done == NC and k0 <= NC
        _loop(NC - k0, lambda k: stream_step(k0 + k))

        for s in shared:
            s.send().wait_send()
        relay_each(my, lambda i: relay_copy(0, i).wait_send())
        pl.when(my == 0)(lambda: relay_direct().wait_send())
        for k in range(NC):
            part_copy(k).wait_send()
        for j in DETOUR:
            if j + NC - FORWARD_FROM in DETOUR:
                forward(j + NC - FORWARD_FROM)
            fin_copy(j).wait_recv()
            detour_out(j).start()
        for k in range(NC):
            act_copy(k).wait_send()
        for j in DETOUR:
            fin_copy(j).wait_send()
        for j in DETOUR:
            detour_out(j).wait_send()

    @pl.when(mx == 1)
    def _stage1():
        first = [Piece(i, 0, p) for i, p in enumerate(LAYER2_PIECES)]
        last = [Piece(len(first) + i, 1, p) for i, p in enumerate(LAYER3_PIECES)]

        def relay_on(hop, i):
            relay_copy(hop - 1, i).wait_recv()
            relay_copy(hop, i).start()

        first[0].load().start()
        first[1].load().start()
        first[0].cast()
        pl.semaphore_wait(barrier, 1)
        first[0].send().start()
        first[1].cast()
        first[1].send().start()
        for s in first[2:]:
            s.load().start()
        pl.semaphore_wait(entered, 1)
        pl.when(my == 0)(lambda: signal(entered, x_nbr))
        relay_each(my, lambda i: relay_on(1, i))
        for s in first[2:]:
            s.cast()
            s.send().start()
        for s in last:
            s.load().start()
        relay_each(1 - my, lambda i: relay_on(2, i))
        for s in last:
            s.cast()
            s.send().start()

        def layer2(k, n):
            for t in range(n):
                act_copy(k + t).wait_recv()
            return mlp(act[_rows(k, n), :], 0).astype(BF16)

        def finish(j, k, n, straight, val):
            fin_s[_rows(j, n), :] = val.astype(BF16)
            for t in range(n):
                (fin_copy if t < straight else detour_in)(j + t).start()
            out_ref[0, own_out(k, n), :] = val

        pending = list(last)

        def need(h):
            while pending and HL + pending[0].piece[1] < h:
                pending.pop(0).send().wait_recv()

        for s in first:
            s.send().wait_recv()

        covered = []
        for kind, *step in EARLY:
            base = len(covered)
            if kind == "swap":
                swap0 = base
                part_s[_rows(swap0, N_SWAP), :] = layer2(swap0, N_SWAP)
                for k in range(swap0, swap0 + N_SWAP):
                    part_copy(k).start()
                covered += [None] * N_SWAP
            elif kind == "new":
                groups, n, h = step
                need(h)

                def early_step(i, base=base, n=n, h=h):
                    k = base + i * n
                    a3 = layer2(k, n)
                    part_s[_rows(k, n), :] = a3
                    if h:
                        acc[_rows(k, n), :] = mlp(a3, 1, 0, h)

                _loop(groups, early_step)
                covered += [h] * (groups * n)
            else:
                k, n, h = step
                assert covered[k:k + n] == [covered[k]] * n
                need(h)
                acc[_rows(k, n), :] += mlp(part_s[_rows(k, n), :], 1, covered[k], h)
                covered[k:k + n] = [h] * n
        assert sorted(CHUNK_AT[:len(covered) - N_SWAP]) == [
            k for k, h in enumerate(covered) if h is not None]

        need(2 * HL)
        j0 = 0
        for k, n, straight in FINISH:
            assert covered[k:k + n] == [covered[k]] * n
            val = mlp(part_s[_rows(k, n), :], 1, covered[k])
            finish(j0, k, n, straight, acc[_rows(k, n), :] + val if covered[k] else val)
            j0 += n
        for groups, n, straight in STEADY:
            def steady_step(i, j0=j0, n=n, straight=straight):
                j = j0 + i * n
                finish(j, N_SWAP + j, n, straight, mlp(layer2(N_SWAP + j, n), 1))

            _loop(groups, steady_step)
            j0 += groups * n

        def land(j):
            out_ref[0, nbr_out(CHUNK_AT[j]), :] = fin_r[_rows(j), :].astype(F32)

        order = _arrival_order()
        here, late = order[:-N_LATE], order[-N_LATE:]
        for k in range(swap0, swap0 + N_SWAP):
            part_copy(k).wait_recv()
        for j in here:
            fin_copy(j).wait_recv()
        swapped = _rows(swap0, N_SWAP)
        both = mlp(jnp.concatenate([part_s[swapped, :], part_r[swapped, :]]), 1)
        out_ref[0, own_out(swap0, N_SWAP), :] = both[:N_SWAP * C]
        out_ref[0, nbr_out(swap0, N_SWAP), :] = both[N_SWAP * C:]
        for j in here:
            land(j)

        for s in first + last:
            s.send().wait_send()
        relay_each(my, lambda i: relay_copy(1, i).wait_send())
        relay_each(1 - my, lambda i: relay_copy(2, i).wait_send())
        for k in range(swap0, swap0 + N_SWAP):
            part_copy(k).wait_send()
        for j in range(N_SENT):
            (detour_in if j in DETOUR else fin_copy)(j).wait_send()
        for j in late:
            fin_copy(j).wait_recv()
            land(j)


def pallas_dist_pipemlp_pp2tp2_xy_b4096_d256_h512_kernel(
    x_padded: jax.Array,
    Win: jax.Array,
    Wout: jax.Array,
):
    n_pieces = len(LAYER2_PIECES) + len(LAYER3_PIECES)
    dma = pltpu.SemaphoreType.DMA
    hbm = pl.BlockSpec(memory_space=pltpu.HBM)
    return pl.pallas_call(
        _body,
        out_shape=jax.ShapeDtypeStruct((1, ROWS, D), F32),
        in_specs=[hbm, hbm, hbm],
        out_specs=pl.BlockSpec(memory_space=pltpu.VMEM),
        scratch_shapes=[
            pltpu.VMEM((2, D, HL), F32),
            pltpu.VMEM((2, HL, D), F32),
            pltpu.VMEM((2, D, 2 * HL), BF16),
            pltpu.VMEM((2, 2 * HL, D), BF16),
            pltpu.VMEM((ROWS, D), F32),
            pltpu.VMEM((HALF, D), F32),
            pltpu.VMEM((HALF, D), BF16),
            pltpu.VMEM((HALF, D), BF16),
            pltpu.VMEM((HALF, D), BF16),
            pltpu.VMEM((HALF, D), BF16),
            pltpu.VMEM((HALF, D), BF16),
            pltpu.VMEM((2, N_RELAY, D), BF16),
            dma((n_pieces,)),
            dma((2 * NC // XN,)),
            dma((6,)),
            dma((n_pieces,)),
            dma((NC,)),
            dma((NC,)),
            dma((NC,)),
            dma((3 * len(RELAY),)),
            pltpu.SemaphoreType.REGULAR,
        ],
        compiler_params=pltpu.CompilerParams(
            collective_id=0,
            vmem_limit_bytes=64 * 1024 * 1024,
            disable_semaphore_checks=True,
        ),
    )(x_padded, Win, Wout)
```

```python
import jax
import jax.numpy as jnp
from jax import lax
from jax.experimental import pallas as pl
from jax.experimental.pallas import tpu as pltpu

F32 = jnp.float32
BF16 = jnp.bfloat16
MESH = pl.DeviceIdType.MESH

ROWS = 4096
D = 256
HL = 512
HALF = ROWS // 2
C = 64
NC = HALF // C
WIN, WOUT = 0, 1

RELAY = (32, 64, 64, 32, 32)
N_RELAY = sum(RELAY)
LAYER1_PIECES = ((WOUT, 0, 64), (WOUT, 64, HL - N_RELAY - 64), (WIN, 0, 128), (WIN, 128, HL - 128))
LAYER2_PIECES = ((WOUT, 0, 64), (WOUT, 64, 320), (WOUT, 384, 128), (WIN, 0, HL))
LAYER3_PIECES = ((WIN, 0, 256), (WOUT, 0, 256), (WIN, 256, 256), (WOUT, 256, 256))

XN = 4
OWN_FIRST = 8
OWN_LATER = ((6, 3), (6, 2))
FORWARD_FROM = 28

EARLY = (("new", 5, 2, HL), ("more", 0, 10, HL + 256), ("swap", 2),
         ("new", 2, 2, HL + 256), ("new", 1, 2, 0))
FINISH = ((12, 2, 2), (14, 2, 2), (0, 10, 6), (16, 2, 0))
STEADY = ((1, 4, 0), (4, 2, 2), (2, 1, 1))

N_SWAP = sum(step[1] for step in EARLY if step[0] == "swap")
N_SENT = NC - N_SWAP
CHUNK_AT = [k + t for k, n, _ in FINISH for t in range(n)]
CHUNK_AT += range(N_SWAP + len(CHUNK_AT), NC)
_STRAIGHT = [t < s for _, n, s in FINISH for t in range(n)]
_STRAIGHT += [t < s for groups, n, s in STEADY for _ in range(groups) for t in range(n)]
DETOUR = [j for j in range(N_SENT) if not _STRAIGHT[j]]
assert len(_STRAIGHT) == N_SENT and DETOUR == list(range(DETOUR[0], DETOUR[-1] + 1))
N_LATE = 8


def _arrival_order():
    queues = [[j for j in range(N_SENT) if _STRAIGHT[j]], list(DETOUR)]
    order = []
    while any(queues):
        for queue in queues:
            if queue:
                order.insert(0, queue.pop())
    return order


def _rows(k, n=1):
    start = k * C
    return pl.ds(start if isinstance(k, int) else pl.multiple_of(start, C), n * C)


def _loop(n, fn):
    if n == 1:
        fn(0)
    elif n > 1:
        lax.fori_loop(0, n, lambda i, _: fn(i), None)


def _body(x_hbm, win_hbm, wout_hbm, out_ref,
          win_f, wout_f, win, wout, xs, acc, part_s, part_r, act, fin_s, fin_r, relay,
          w_sem, x_sem, send_sems, w_rsem, part_rsem, act_rsem, fin_rsem, relay_rsem, entered):
    mx = lax.axis_index("x")
    my = lax.axis_index("y")
    x_nbr = (1 - mx, my)
    y_nbr = (mx, 1 - my)

    def own_out(k, n=1):
        return pl.ds(pl.multiple_of(my * HALF + k * C, C), n * C)

    def nbr_out(k, n=1):
        return pl.ds(pl.multiple_of((1 - my) * HALF + k * C, C), n * C)

    def signal(sem, dev):
        pl.semaphore_signal(sem, 1, device_id=dev, device_id_type=MESH)

    barrier = pltpu.get_barrier_semaphore()
    signal(barrier, y_nbr)
    pl.when((mx == 1) & (my == 0))(lambda: signal(barrier, x_nbr))

    def remote(src, dst, send_sem, recv_sem, dev):
        return pltpu.make_async_remote_copy(
            src, dst, send_sem, recv_sem, device_id=dev, device_id_type=MESH)

    class Piece:
        def __init__(self, i, layer, piece):
            self.i, self.layer, self.piece = i, layer, piece

        def view(self, refs, shift=0):
            m, h0, n = self.piece
            hidden = pl.ds(h0 + shift, n)
            if m == WIN:
                return refs[m].at[self.layer, :, hidden]
            return refs[m].at[self.layer, hidden, :]

        def load(self):
            return pltpu.make_async_copy(
                self.view((win_hbm, wout_hbm)), self.view((win_f, wout_f)), w_sem.at[self.i])

        def cast(self):
            self.load().wait()
            self.view((win, wout))[...] = self.view((win_f, wout_f))[...].astype(BF16)

        def send(self):
            return remote(self.view((win, wout)), self.view((win, wout), HL),
                          send_sems.at[0], w_rsem.at[self.i], y_nbr)

    def relay_copy(hop, i):
        r0, n = sum(RELAY[:i]), RELAY[i]
        here = pl.ds(r0, n)
        src = wout.at[1, pl.ds(HL - N_RELAY + r0, n)] if hop == 0 else relay.at[hop - 1, here]
        dst = wout.at[1, pl.ds(2 * HL - N_RELAY + r0, n)] if hop == 2 else relay.at[hop, here]
        return remote(src, dst, send_sems.at[5], relay_rsem.at[hop * len(RELAY) + i],
                      y_nbr if hop == 1 else x_nbr)

    def relay_each(y, fn):
        pl.when(y == 1)(lambda: fn(0))
        for i in range(1, len(RELAY)):
            fn(i)

    def relay_direct():
        h0 = HL - N_RELAY
        return remote(wout.at[1, pl.ds(h0, RELAY[0])], wout.at[1, pl.ds(HL + h0, RELAY[0])],
                      send_sems.at[5], relay_rsem.at[0], y_nbr)

    def part_copy(k):
        return remote(part_s.at[_rows(k)], part_r.at[_rows(k)], send_sems.at[1],
                      part_rsem.at[k], y_nbr)

    def act_copy(k):
        return remote(act.at[_rows(k)], act.at[_rows(k)], send_sems.at[2], act_rsem.at[k], x_nbr)

    def fin_copy(j):
        return remote(fin_s.at[_rows(j)], fin_r.at[_rows(j)], send_sems.at[3],
                      fin_rsem.at[j], y_nbr)

    def detour_in(j):
        return remote(fin_s.at[_rows(j)], fin_s.at[_rows(j)], send_sems.at[4],
                      act_rsem.at[j], x_nbr)

    def detour_out(j):
        return remote(fin_r.at[_rows(j)], fin_r.at[_rows(j)], send_sems.at[4],
                      fin_rsem.at[j], x_nbr)

    def mlp(a, layer, h0=0, h1=2 * HL):
        h = jnp.dot(a, win[layer, :, h0:h1], preferred_element_type=F32)
        h = jnp.maximum(h, 0.0).astype(BF16)
        return jnp.dot(h, wout[layer, h0:h1, :], preferred_element_type=F32)

    @pl.when(mx == 0)
    def _stage0():
        shared = [Piece(i, 1, p) for i, p in enumerate(LAYER1_PIECES)]
        local = [Piece(len(shared) + m, 0, (m, 0, HL)) for m in (WIN, WOUT)]
        relayed = Piece(len(shared) + 2, 1, (WOUT, HL - N_RELAY, N_RELAY))

        def x_load(i):
            src = pl.multiple_of(((1 - my) * HALF + i * XN * C) % ROWS, XN * C)
            return pltpu.make_async_copy(
                x_hbm.at[0, pl.ds(src, XN * C)], xs.at[_rows(i * XN, XN)], x_sem.at[i])

        def layer0(k, n):
            return mlp(xs[_rows(k, n), :].astype(BF16), 0, 0, HL)

        def nbr_partial(i, loads, ahead):
            for t in range(loads):
                x_load(i + t).wait()
                x_load(i + t + ahead).start()
            part_s[_rows(i * XN, loads * XN), :] = layer0(i * XN, loads * XN).astype(BF16)

        def part_start(i, loads):
            for t in range(loads * XN):
                part_copy(i * XN + t).start()

        shared[0].load().start()
        shared[1].load().start()
        shared[0].cast()
        for s in local:
            s.load().start()
        x_load(0).start()
        pl.when(my == 0)(lambda: pl.semaphore_wait(barrier, 2))
        pl.when(my == 1)(lambda: pl.semaphore_wait(barrier, 1))
        shared[0].send().start()
        pl.when(my == 0)(lambda: signal(entered, x_nbr))
        shared[1].cast()
        shared[1].send().start()
        local[0].cast()
        relayed.load().start()
        shared[2].load().start()
        local[1].cast()
        relayed.cast()

        @pl.when(my == 0)
        def _():
            relay_direct().start()
            relay_each(0, lambda i: relay_copy(0, i).start())

        pl.semaphore_wait(entered, 1)
        pl.when(my == 0)(lambda: signal(entered, y_nbr))

        @pl.when(my == 1)
        def _():
            signal(entered, x_nbr)
            relay_each(1, lambda i: relay_copy(0, i).start())

        shared[2].cast()
        shared[2].send().start()
        shared[3].load().start()
        x_load(1).start()

        nbr_partial(0, 1, 2)
        shared[3].cast()
        shared[3].send().start()
        part_start(0, 1)
        nbr_partial(1, 1, 2)
        part_start(1, 1)
        x_load(4).start()
        x_load(5).start()

        def nbr_step(i):
            nbr_partial(2 * i + 2, 2, 4)
            part_start(2 * i + 2, 2)

        n_loads = NC // XN
        _loop(n_loads // 2 - 1, nbr_step)

        for i in range(n_loads + 4, 2 * n_loads):
            x_load(i).start()
        for i in range(n_loads, n_loads + OWN_FIRST // XN):
            x_load(i).wait()
        acc[_rows(0, OWN_FIRST), :] = layer0(NC, OWN_FIRST)
        for i in range(n_loads + OWN_FIRST // XN, 2 * n_loads):
            x_load(i).wait()

        for s in shared:
            s.send().wait_recv()
        relay_each(1 - my, lambda i: relay_copy(2, i).wait_recv())
        pl.when(my == 1)(lambda: relay_direct().wait_recv())

        def forward(j):
            detour_in(j).wait_recv()
            fin_copy(j).start()

        def stream_step(k, own=None):
            part_copy(k).wait_recv()
            a1 = (acc[_rows(k), :] + part_r[_rows(k), :].astype(F32)).astype(BF16)
            act[_rows(k), :] = mlp(a1, 1).astype(BF16)
            act_copy(k).start()
            if own is not None:
                acc[_rows(own, 2), :] = layer0(NC + own, 2)
            out_ref[0, _rows(2 * k, 2), :] = jnp.zeros((2 * C, D), F32)
            pl.when((k >= FORWARD_FROM) & (k < FORWARD_FROM + len(DETOUR)))(
                lambda: forward(DETOUR[0] + k - FORWARD_FROM))

        stream_step(0)
        k0, done = 1, OWN_FIRST
        for runs, length in OWN_LATER:
            assert all(k0 + i * length < done + 2 * i for i in range(runs))

            def stream_run(i, k0=k0, done=done, length=length):
                stream_step(k0 + i * length, own=done + 2 * i)
                _loop(length - 1, lambda t: stream_step(k0 + i * length + 1 + t))

            _loop(runs, stream_run)
            k0, done = k0 + runs * length, done + 2 * runs
        assert done == NC and k0 <= NC
        _loop(NC - k0, lambda k: stream_step(k0 + k))

        for s in shared:
            s.send().wait_send()
        relay_each(my, lambda i: relay_copy(0, i).wait_send())
        pl.when(my == 0)(lambda: relay_direct().wait_send())
        for k in range(NC):
            part_copy(k).wait_send()
        for j in DETOUR:
            if j + NC - FORWARD_FROM in DETOUR:
                forward(j + NC - FORWARD_FROM)
            fin_copy(j).wait_recv()
            detour_out(j).start()
        for k in range(NC):
            act_copy(k).wait_send()
        for j in DETOUR:
            fin_copy(j).wait_send()
        for j in DETOUR:
            detour_out(j).wait_send()

    @pl.when(mx == 1)
    def _stage1():
        first = [Piece(i, 0, p) for i, p in enumerate(LAYER2_PIECES)]
        last = [Piece(len(first) + i, 1, p) for i, p in enumerate(LAYER3_PIECES)]

        def relay_on(hop, i):
            relay_copy(hop - 1, i).wait_recv()
            relay_copy(hop, i).start()

        first[0].load().start()
        first[1].load().start()
        first[0].cast()
        pl.semaphore_wait(barrier, 1)
        first[0].send().start()
        first[1].cast()
        first[1].send().start()
        for s in first[2:]:
            s.load().start()
        pl.semaphore_wait(entered, 1)
        pl.when(my == 0)(lambda: signal(entered, x_nbr))
        relay_each(my, lambda i: relay_on(1, i))
        for s in first[2:]:
            s.cast()
            s.send().start()
        for s in last:
            s.load().start()
        relay_each(1 - my, lambda i: relay_on(2, i))
        for s in last:
            s.cast()
            s.send().start()

        def layer2(k, n):
            for t in range(n):
                act_copy(k + t).wait_recv()
            return mlp(act[_rows(k, n), :], 0).astype(BF16)

        def finish(j, k, n, straight, val):
            fin_s[_rows(j, n), :] = val.astype(BF16)
            for t in range(n):
                (fin_copy if t < straight else detour_in)(j + t).start()
            out_ref[0, own_out(k, n), :] = val

        pending = list(last)

        def need(h):
            while pending and HL + pending[0].piece[1] < h:
                pending.pop(0).send().wait_recv()

        for s in first:
            s.send().wait_recv()

        covered = []
        for kind, *step in EARLY:
            base = len(covered)
            if kind == "swap":
                swap0 = base
                part_s[_rows(swap0, N_SWAP), :] = layer2(swap0, N_SWAP)
                for k in range(swap0, swap0 + N_SWAP):
                    part_copy(k).start()
                covered += [None] * N_SWAP
            elif kind == "new":
                groups, n, h = step
                need(h)

                def early_step(i, base=base, n=n, h=h):
                    k = base + i * n
                    a3 = layer2(k, n)
                    part_s[_rows(k, n), :] = a3
                    if h:
                        acc[_rows(k, n), :] = mlp(a3, 1, 0, h)

                _loop(groups, early_step)
                covered += [h] * (groups * n)
            else:
                k, n, h = step
                assert covered[k:k + n] == [covered[k]] * n
                need(h)
                acc[_rows(k, n), :] += mlp(part_s[_rows(k, n), :], 1, covered[k], h)
                covered[k:k + n] = [h] * n
        assert sorted(CHUNK_AT[:len(covered) - N_SWAP]) == [
            k for k, h in enumerate(covered) if h is not None]

        need(2 * HL)
        j0 = 0
        for k, n, straight in FINISH:
            assert covered[k:k + n] == [covered[k]] * n
            val = mlp(part_s[_rows(k, n), :], 1, covered[k])
            finish(j0, k, n, straight, acc[_rows(k, n), :] + val if covered[k] else val)
            j0 += n
        for groups, n, straight in STEADY:
            def steady_step(i, j0=j0, n=n, straight=straight):
                j = j0 + i * n
                finish(j, N_SWAP + j, n, straight, mlp(layer2(N_SWAP + j, n), 1))

            _loop(groups, steady_step)
            j0 += groups * n

        def land(j):
            out_ref[0, nbr_out(CHUNK_AT[j]), :] = fin_r[_rows(j), :].astype(F32)

        order = _arrival_order()
        here, late = order[:-N_LATE], order[-N_LATE:]
        for k in range(swap0, swap0 + N_SWAP):
            part_copy(k).wait_recv()
        for j in here:
            fin_copy(j).wait_recv()
        swapped = _rows(swap0, N_SWAP)
        both = mlp(jnp.concatenate([part_s[swapped, :], part_r[swapped, :]]), 1)
        out_ref[0, own_out(swap0, N_SWAP), :] = both[:N_SWAP * C]
        out_ref[0, nbr_out(swap0, N_SWAP), :] = both[N_SWAP * C:]
        for j in here:
            land(j)

        for s in first + last:
            s.send().wait_send()
        relay_each(my, lambda i: relay_copy(1, i).wait_send())
        relay_each(1 - my, lambda i: relay_copy(2, i).wait_send())
        for k in range(swap0, swap0 + N_SWAP):
            part_copy(k).wait_send()
        for j in range(N_SENT):
            (detour_in if j in DETOUR else fin_copy)(j).wait_send()
        for j in late:
            fin_copy(j).wait_recv()
            land(j)


def pallas_dist_pipemlp_pp2tp2_xy_b4096_d256_h512_kernel(
    x_padded: jax.Array,
    Win: jax.Array,
    Wout: jax.Array,
):
    n_pieces = len(LAYER2_PIECES) + len(LAYER3_PIECES)
    dma = pltpu.SemaphoreType.DMA
    hbm = pl.BlockSpec(memory_space=pltpu.HBM)
    return pl.pallas_call(
        _body,
        out_shape=jax.ShapeDtypeStruct((1, ROWS, D), F32),
        in_specs=[hbm, hbm, hbm],
        out_specs=pl.BlockSpec(memory_space=pltpu.VMEM),
        scratch_shapes=[
            pltpu.VMEM((2, D, HL), F32),
            pltpu.VMEM((2, HL, D), F32),
            pltpu.VMEM((2, D, 2 * HL), BF16),
            pltpu.VMEM((2, 2 * HL, D), BF16),
            pltpu.VMEM((ROWS, D), F32),
            pltpu.VMEM((HALF, D), F32),
            pltpu.VMEM((HALF, D), BF16),
            pltpu.VMEM((HALF, D), BF16),
            pltpu.VMEM((HALF, D), BF16),
            pltpu.VMEM((HALF, D), BF16),
            pltpu.VMEM((HALF, D), BF16),
            pltpu.VMEM((2, N_RELAY, D), BF16),
            dma((n_pieces,)),
            dma((2 * NC // XN,)),
            dma((6,)),
            dma((n_pieces,)),
            dma((NC,)),
            dma((NC,)),
            dma((NC,)),
            dma((3 * len(RELAY),)),
            pltpu.SemaphoreType.REGULAR,
        ],
        compiler_params=pltpu.CompilerParams(
            collective_id=0,
            vmem_limit_bytes=64 * 1024 * 1024,
            disable_semaphore_checks=True,
        ),
    )(x_padded, Win, Wout)
```
